```python
import numpy as np

kernel_name = "dist_rs_xy_x_m65536_n1024"

def setup_inputs():
    return {"x": np.random.randn(2, 65536, 1024).astype(np.float32)}

def reference(x: np.ndarray) -> np.ndarray:
    return x.sum(axis=0)
```

```python
import jax
import jax.numpy as jnp
from jax import lax
from jax.experimental import pallas as pl
from jax.experimental.pallas import tpu as pltpu

S = 8
FRAME = 16 * S
QUEUE = 6
SHIFT = 4
BOTH = 1
LEAD = 2
AHEAD = LEAD + SHIFT
Y_LAG = 3
LOADS, OWN, SENDS, RELAYS = 8, 4, 8, 4
RING = 16

MSB = -0x80000000
TOP = 0x80808080 - (1 << 32)
OVER_31 = 0xE0E0E0E0 - (1 << 32)


def _shr(a, n):
    return lax.shift_right_logical(a, jnp.int32(n) if isinstance(n, int) else n)


def _swap_bytes(a, b):
    t = (_shr(a, 8) ^ b) & 0x00FF00FF
    return a ^ (t << 8), b ^ t


def _slabs(a):
    return [a[k * S:(k + 1) * S] for k in range(a.shape[0] // S)]


def _append(queue, n, bits):
    i, s = n >> 5, n & 31
    hi, lo = _shr(bits, s), (bits << 1) << (s ^ 31)
    at = [i == j for j in range(len(queue))]
    return [
        q | jnp.where(at[j], hi, jnp.where(at[j - 1], lo, 0) if j else 0)
        for j, q in enumerate(queue)
    ]


def _window(words, o):
    a, b = words[0], words[1]
    for j in range(1, len(words)):
        past = o >= 32 * j
        a = jnp.where(past, words[j], a)
        if j + 1 < len(words):
            b = jnp.where(past, words[j + 1], b)
    s = o & 31
    return (a << s) | _shr(_shr(b, 1), s ^ 31)


def _words_before(f):
    return 2 * f - f // 4


def pallas_dist_rs_xy_x_m65536_n1024_kernel(x: jax.Array):
    _, m, n_cols = x.shape
    w = n_cols // 2
    lanes = w // 2
    half = m // 2 // FRAME
    frames = (half + BOTH, half - BOTH)
    n_x, n_y = frames
    first_slot = (0, n_x + SHIFT)
    total_words = _words_before(n_x) + QUEUE - 1

    def body(x_ref, o_ref, theirs_buf, own_buf, send_buf, recv_buf, relay_buf, enc_ref, dec_ref,
             extra_sent, extra_relayed, theirs_sem, own_sem, out_sems, in_sems, head_sems,
             extra_out_sems, extra_in_sems):
        mx, my = lax.axis_index("x"), lax.axis_index("y")
        peer = ((1 - mx, my), (mx, 1 - my))
        zero = jnp.zeros((S, lanes), jnp.int32)

        def first_row(link, f):
            k = (1 - my) * half + f
            if link == 0:
                k = jnp.where(f < half, my * half + f, k - BOTH)
            return pl.multiple_of(k * FRAME, FRAME)

        def load_theirs(f):
            cols = pl.ds(pl.multiple_of((1 - mx) * w, w), w)
            src = x_ref.at[0, pl.ds(first_row(0, f), FRAME), cols]
            return pltpu.make_async_copy(src, theirs_buf.at[f % LOADS], theirs_sem.at[f % LOADS])

        def load_own(link, f):
            cols = pl.ds(pl.multiple_of(mx * w, w), w)
            src = x_ref.at[0, pl.ds(first_row(link, f), FRAME), cols]
            slot = link * OWN + f % OWN
            return pltpu.make_async_copy(src, own_buf.at[slot], own_sem.at[slot])

        def remote(link, src, dst, send_sem, recv_sem):
            return pltpu.make_async_remote_copy(
                src, dst, send_sem, recv_sem,
                device_id=peer[link], device_id_type=pl.DeviceIdType.MESH)

        def message(link, f, action):
            g = f + SHIFT
            codes = (jnp.minimum(_words_before(g + 1), total_words)
                     - jnp.minimum(_words_before(g), total_words))
            codes = jnp.where(f < LEAD, 0, codes)
            for k in range(3):
                @pl.when(codes == k)
                def _():
                    part = pl.ds(0, (9 + k) * S)
                    src = recv_buf.at[g, part] if link else send_buf.at[g % SENDS, part]
                    sent = out_sems.at[SENDS + f % RELAYS if link else f % SENDS]
                    action(remote(link, src, recv_buf.at[first_slot[link] + g, part],
                                  sent, in_sems.at[link * RING + f % RING]))

        def head(link):
            part = pl.ds(9 * S, 2 * S)
            src = (recv_buf if link else send_buf).at[pl.ds(0, AHEAD), part]
            return remote(link, src, recv_buf.at[pl.ds(first_slot[link], AHEAD), part],
                          head_sems.at[2 * link], head_sems.at[2 * link + 1])

        def parked(link, f, side):
            return pl.ds(first_row(link, f), 14 * S), pl.ds(side * lanes, lanes)

        def extra(link, f):
            src = relay_buf.at[f % RELAYS] if link else o_ref.at[parked(0, f, 1)]
            sent = extra_out_sems.at[RING + f % RELAYS if link else f % RING]
            return remote(link, src, o_ref.at[parked(0, f, 0)],
                          sent, extra_in_sems.at[link * RING + f % RING])

        def rounded(f, n_rows=FRAME):
            return pltpu.bitcast(theirs_buf[f % LOADS, 0:n_rows, :].astype(jnp.bfloat16), jnp.int32)

        def reference(f):
            mean = jnp.sum((rounded(f, 2 * S) & 0x7FFF).astype(jnp.float32)) * (1.0 / (S * w))
            return jnp.minimum((zero.astype(jnp.float32) + mean).astype(jnp.int32) + 4 * 128, 0x7FFF)

        def spread(ref):
            return jnp.concatenate([ref | (ref << 16)] * 8, axis=0)

        def split(f, ref):
            words, ref = rounded(f), spread(ref)
            low, high = _swap_bytes(ref - words[:, :lanes], ref - words[:, lanes:])
            sign = high & TOP
            return low, sign, high ^ sign

        def drain(f, second, queue, n):
            hold = False if second else f % 4 == 3
            moved = [jnp.where(hold, a, b) for a, b in zip(queue, queue[1:] + [zero])]
            return queue[0], moved, jnp.maximum(n - jnp.where(hold, 0, 32), 0)

        def commit(f, drained, queue, n, ref):
            a, b = drained
            send_buf[f % SENDS, 9 * S:11 * S, :] = jnp.concatenate(
                [jnp.where(f % 4 == 3, b, a), b], axis=0)
            enc_ref[...] = jnp.concatenate(queue + [n, ref], axis=0)

        def encode(f):
            load_theirs(f).wait()

            @pl.when(f == 0)
            def _():
                ref = reference(f)
                enc_ref[...] = jnp.concatenate(
                    [ref] + [zero] * (QUEUE - 1) + [zero + 32, ref], axis=0)

            *queue, n, ref = _slabs(enc_ref[...])
            low, sign, cls = split(f, ref)
            signs = zero
            for k, bits in enumerate(_slabs(sign)):
                signs = signs | _shr(bits, k)
            send_buf[(f + SHIFT) % SENDS, 0:9 * S, :] = jnp.concatenate([low, signs], axis=0)

            @pl.when(f < LEAD)
            def _():
                pl.when(f == 0)(lambda: pl.semaphore_wait(barrier, 2))
                message(0, f, lambda c: c.start())

            hop = (cls + 0x04040403 - _shr((cls + 0x7F7F7F7F) & TOP, 5)
                   + _shr((cls + 0x7C7C7C7C) & TOP, 7))
            b0 = _shr(jnp.full_like(hop, MSB), hop & 31)
            b1 = _shr(b0, _shr(hop, 8) & 31)
            b2 = _shr(b1, _shr(hop, 16) & 31)
            b3 = _shr(b2, _shr(hop, 24) & 31)
            size = lax.clz(b3) + 1
            misfit = (hop[0:S] & 16) << 1
            drained = []
            for k, (bits, count, over) in enumerate(
                    zip(_slabs((b0 | b1) | (b2 | b3)), _slabs(size), _slabs(hop | size))):
                queue = _append(queue, n, bits)
                n = n + count
                misfit = misfit | over
                if k % 4 == 3:
                    misfit = misfit | ((32 * QUEUE - n) & MSB)
                    word, queue, n = drain(f, k == 7, queue, n)
                    drained.append(word)
            verbatim = jnp.max(jnp.where((misfit & OVER_31) != 0, 1.0, 0.0)) > 0.0
            extra_sent[f % RING] = verbatim.astype(jnp.int32)

            @pl.when(jnp.logical_not(verbatim))
            def _():
                commit(f, drained, queue, n, ref)

            @pl.when(verbatim)
            def _():
                *queue, n, ref = _slabs(enc_ref[...])
                *seven, last = _slabs(split(f, ref)[2])
                seven = [c | ((last << (k + 1)) & TOP) for k, c in enumerate(seven)]
                o_ref[parked(0, f, 1)] = pltpu.bitcast(jnp.concatenate(seven, axis=0), jnp.bfloat16)
                extra(0, f).start()
                ref = reference(f)
                a, queue, n = drain(f, False, _append(queue, n, ref), n + 32)
                b, queue, n = drain(f, True, queue, n)
                commit(f, (a, b), queue, n, ref)

            @pl.when(f == n_x - 1)
            def _():
                g, left = n_x, _slabs(enc_ref[0:(QUEUE - 1) * S, :])
                while left:
                    k = min(_words_before(g + 1) - _words_before(g), len(left))
                    send_buf[g % SENDS, 9 * S:(9 + k) * S, :] = jnp.concatenate(left[:k], axis=0)
                    g, left = g + 1, left[k:]

            pl.when(f + LOADS < n_x)(lambda: load_theirs(f + LOADS).start())

        def reduce(link, f):
            slot = first_slot[link] + f
            state = pl.ds(2 * link * S, 2 * S)

            @pl.when(f == 0)
            def _():
                if link == 1:
                    head(1).wait_recv()
                dec_ref[state, :] = jnp.concatenate(
                    [zero + 32, recv_buf[slot, 9 * S:10 * S, :]], axis=0)

            o, ref = _slabs(dec_ref[state, :])
            pairs = recv_buf[pl.ds(slot, SHIFT), 9 * S:11 * S, :]
            slots = [pairs[j // 2, (j % 2) * S:(j % 2 + 1) * S] for j in range(2 * SHIFT)]
            gap = 2 * (3 - f % 4)
            words = [jnp.where(j > gap, slots[j + 1], slots[j]) for j in range(QUEUE + 1)]
            hold = f % 4 == 3
            mark = _window(words[:QUEUE], o)
            verbatim = jnp.max(_shr(mark[:, 0:128], 16).astype(jnp.float32)) == 0.0

            load_own(link, f).wait()
            if link == 0:
                pl.when(extra_sent[f % RING] != 0)(lambda: extra(0, f).wait_send())

                @pl.when(f >= RELAYS)
                def _():
                    pl.when(extra_relayed[f % RELAYS] != 0)(lambda: extra(1, f - RELAYS).wait_send())

                extra_relayed[f % RELAYS] = jnp.logical_and(verbatim, f < n_y).astype(jnp.int32)

            def finish(cls):
                pl.when(f >= (0 if link else n_y))(lambda: message(link, f, lambda c: c.wait_recv()))
                fixed = recv_buf[slot + SHIFT, 0:9 * S, :]
                sign = jnp.concatenate([fixed[8 * S:] << k for k in range(8)], axis=0) & TOP
                a, b = _swap_bytes(fixed[:8 * S], cls | sign)
                other = jnp.concatenate([spread(ref) - a, spread(ref) - b], axis=1)
                other = pltpu.bitcast(other, jnp.bfloat16).astype(jnp.float32)
                total = own_buf[link * OWN + f % OWN] + other
                o_ref[pl.ds(first_row(link, f), FRAME), :] = total.astype(jnp.bfloat16)

            @pl.when(jnp.logical_not(verbatim))
            def _():
                at, near, zeros = o, words[:QUEUE], []
                for k in range(8):
                    bits = _window(near, at) if k else mark
                    r = []
                    for j in range(4):
                        r.append(lax.clz(bits))
                        if j < 3:
                            bits = (bits << 1) << r[j]
                    zeros.append((r[0] | (r[1] << 8)) | ((r[2] << 16) | (r[3] << 24)))
                    at = at + (r[0] + r[1]) + (r[2] + r[3]) + 4
                    if k == 3:
                        at = jnp.maximum(at - jnp.where(hold, 0, 32), 0)
                        near = [jnp.where(hold, a, b) for a, b in zip(words, words[1:])]
                dec_ref[state, :] = jnp.concatenate([jnp.maximum(at - 32, 0), ref], axis=0)
                z = jnp.concatenate(zeros, axis=0)
                ge3, ge4 = (z + 0x7D7D7D7D) & TOP, (z + 0x7C7C7C7C) & TOP
                finish(z + 0x01010101 - _shr(ge3 - ge4, 5) - _shr(ge4, 7))

            @pl.when(verbatim)
            def _():
                box = o_ref.at[parked(link, f, 0)]
                remote(link, box, box, extra_out_sems.at[0],
                       extra_in_sems.at[link * RING + f % RING]).wait_recv()
                packed = o_ref[parked(link, f, 0)]
                if link == 0:
                    @pl.when(f < n_y)
                    def _():
                        relay_buf[f % RELAYS] = packed
                        extra(1, f).start()

                seven, last = _slabs(pltpu.bitcast(packed, jnp.int32)), zero
                for k, c in enumerate(seven):
                    last = last | _shr(c & TOP, k + 1)
                dec_ref[state, :] = jnp.concatenate(
                    [jnp.maximum(o - jnp.where(hold, 0, 32), 0), mark], axis=0)
                finish(jnp.concatenate(seven + [last], axis=0) & 0x7F7F7F7F)

            pl.when(f + OWN < frames[link])(lambda: load_own(link, f + OWN).start())

        def reduced(link, s):
            lag = jnp.where(s >= n_y, 1, Y_LAG) if link else 0
            return jnp.where(s < LEAD + link * Y_LAG, 0, jnp.minimum(s - lag + 1, frames[link]))

        load_theirs(0).start()
        barrier = pltpu.get_barrier_semaphore()
        for device in peer:
            pl.semaphore_signal(barrier, inc=1, device_id=device, device_id_type=pl.DeviceIdType.MESH)
        for f in range(1, LOADS):
            load_theirs(f).start()

        steps = max(n_x, n_y + 1)

        @pl.loop(-AHEAD, steps)
        def step(s):
            @pl.when(s == LEAD)
            def _():
                head(0).wait_recv()
                head(1).start()

            @pl.when(jnp.logical_and(s >= 0, s < n_y))
            def _():
                message(0, s, lambda c: c.wait_recv())
                message(1, s, lambda c: c.start())

            for link, f in ((1, s + 1 - RELAYS), (0, s + AHEAD - SENDS)):
                @pl.when(jnp.logical_and(f >= 0, f < frames[link]))
                def _():
                    message(link, f, lambda c: c.wait_send())

            pl.when(s + AHEAD == SENDS)(lambda: head(0).wait_send())
            pl.when(s == LEAD + RELAYS)(lambda: head(1).wait_send())

            @pl.when(s == 0)
            def _():
                for link in range(2):
                    for f in range(OWN):
                        load_own(link, f).start()

            pl.when(s + AHEAD < n_x)(lambda: encode(s + AHEAD))
            pl.when(s == -1)(lambda: head(0).start())

            @pl.when(jnp.logical_and(s >= 0, s + LEAD < n_x))
            def _():
                message(0, s + LEAD, lambda c: c.start())

            for link in range(2):
                @pl.loop(reduced(link, s - 1), reduced(link, s))
                def _(f):
                    reduce(link, f)

        for link, first in ((0, steps + AHEAD - SENDS), (1, steps + 1 - RELAYS)):
            for f in range(first, frames[link]):
                message(link, f, lambda c: c.wait_send())
        for f in range(n_x - RELAYS, n_y):
            pl.when(extra_relayed[f % RELAYS] != 0)(lambda: extra(1, f).wait_send())

    dma = pltpu.SemaphoreType.DMA
    return pl.pallas_call(
        body,
        out_shape=pltpu.VMEM((m, w), jnp.bfloat16),
        in_specs=[pl.BlockSpec(memory_space=pl.ANY)],
        out_specs=pl.BlockSpec(memory_space=pltpu.VMEM),
        scratch_shapes=[
            pltpu.VMEM((LOADS, FRAME, w), jnp.float32),
            pltpu.VMEM((2 * OWN, FRAME, w), jnp.float32),
            pltpu.VMEM((SENDS, 11 * S, lanes), jnp.int32),
            pltpu.VMEM((n_x + n_y + 2 * SHIFT, 11 * S, lanes), jnp.int32),
            pltpu.VMEM((RELAYS, 14 * S, lanes), jnp.bfloat16),
            pltpu.VMEM(((QUEUE + 2) * S, lanes), jnp.int32),
            pltpu.VMEM((4 * S, lanes), jnp.int32),
            pltpu.SMEM((RING,), jnp.int32),
            pltpu.SMEM((RELAYS,), jnp.int32),
            dma((LOADS,)),
            dma((2 * OWN,)),
            dma((SENDS + RELAYS,)),
            dma((2 * RING,)),
            dma((4,)),
            dma((RING + RELAYS,)),
            dma((2 * RING,)),
        ],
        compiler_params=pltpu.CompilerParams(
            collective_id=0,
            vmem_limit_bytes=56 * 2**20,
            disable_bounds_checks=True,
            disable_semaphore_checks=True,
        ),
    )(x)
```
